```python
import numpy as np

kernel_name = "dist_sparse_attn_strided_qseq_b1_sq1024_skv1024_hq8_dh128"

def setup_inputs():
    x = np.random.randn(1, 4096, 1024).astype(np.float32)
    Wq = np.random.randn(1024, 4096).astype(np.float32) * 0.02
    K_ext = np.random.randn(1, 1024, 32, 128).astype(np.float32)
    V_ext = np.random.randn(1, 1024, 32, 128).astype(np.float32)
    Wo = np.random.randn(4096, 1024).astype(np.float32) * 0.02
    return {"x": x, "Wq": Wq, "K_ext": K_ext, "V_ext": V_ext, "Wo": Wo}

def reference(x, Wq, K_ext, V_ext, Wo):
    B, Sq, Skv, Hq, Dh = 1, 4096, 1024, 32, 128
    Q = (x @ Wq).reshape(B, Sq, Hq, Dh)
    qb = (np.arange(Sq) // 64)[:, None]
    kb = (np.arange(Skv) // 64)[None, :]
    mask = (qb == kb) | ((kb % 4) == (qb % 4))
    scores = np.einsum('bihd,bjhd->bhij', Q, K_ext).astype(np.float32) * 0.08838834764831843
    scores = np.where(mask[None, None, :, :], scores, -1e9)
    scores_max = scores.max(axis=-1, keepdims=True)
    w = np.exp(scores - scores_max)
    row_keep = mask.any(axis=1)
    w_sum = np.where(row_keep[None, None, :, None], w.sum(axis=-1, keepdims=True), 1.0)
    w = w / w_sum
    w = np.where(row_keep[None, None, :, None], w, 0.0)
    ctx = np.einsum('bhij,bjhd->bihd', w, V_ext).reshape(B, Sq, Hq * Dh)
    return ctx @ Wo
```

```python
import jax
import jax.numpy as jnp
from jax import lax
from jax.experimental import pallas as pl
from jax.experimental.pallas import tpu as pltpu

SCALE = 0.08838834764831843
LOG2E = 1.4426950408889634
_NT = (((1,), (1,)), ((), ()))
bf16 = jnp.bfloat16
f32 = jnp.float32
MESH = pl.DeviceIdType.MESH


def _code(s, k, c):
    return s * 64 + k * 4 + c


def _t1(ks, cs=range(4)):
    return [_code(0, k, c) for k in ks for c in cs]


def _t2(c, ks=range(8)):
    return [_code(1, k, c) for k in ks]


def _t3(ks, cs=range(4)):
    return [_code(0, 8 + k, c) for k in ks for c in cs]


def _t4(cs, ks):
    return [_code(1, 8 + k, c) for c in cs for k in ks]


_STAGES = [
    ([], [], [(0, 0)]),
    ([], [1], [(1, 0)]),
    ([1], [], [(0, 1), (1, 1)]),
    ([], [2], [(2, 0), (2, 1)]),
    ([], [3], [(3, 0), (3, 1)]),
    ([2], [], [(0, 2), (1, 2), (2, 2)]),
    ([], [4], [(3, 2), (4, 0), (4, 1)]),
    ([], [5, 6], [(4, 2), (5, 0), (5, 1), (5, 2), (6, 0), (6, 1)]),
    ([3], [7], [(6, 2), (7, 0), (7, 1), (7, 2), (0, 3), (1, 3), (2, 3), (3, 3)]),
]
_Q_PRO = [_code(0, k, c) for _, _, us in _STAGES for k, c in us]
_Q_MAIN = [
    (_t1([4, 5, 6, 7], [3]), _t3([0])),
    (_t2(0, range(4)), _t2(0, range(4, 8))),
    (_t3([1]), _t3([2])),
    (_t4([0], range(4)), _t2(1, range(4))),
    (_t2(1, range(4, 8)), _t4([1], range(4))),
    (_t4([0, 1], [4]) + _t3([3], [0, 1]), _t3([3], [2, 3]) + _t3([4], [0, 1])),
    (_t2(2, range(4)), _t2(2, range(4, 8))),
    (_t4([2], range(4)), _t4([2], [4, 5]) + _t4([0, 1], [5])),
    (_t4([0, 1, 2], [6]) + _t3([4], [2]), _t3([4], [3]) + _t3([5], [0, 1, 2])),
    (_t4([0, 1, 2], [7]) + _t2(3, [0]), _t2(3, [1, 2, 3, 4])),
    (_t2(3, [5, 6, 7]) + _t4([3], [0]), _t4([3], [1, 2, 3, 4])),
    (_t4([3], [5, 6, 7]) + _t3([5], [3]), _t3([6])),
]
_Q_TAIL = _t3([7])
_A_MAIN = [
    (_t1([0]), _t1([1])),
    (_t1([2]), _t1([3])),
    (_t2(0, range(4, 8)), _t2(0, range(4))),
    (_t1([4], [0, 1, 2]) + _t1([5], [0]), _t1([4, 5, 6, 7], [3])),
    (_t2(1, range(4)), _t2(1, range(4, 8))),
    (_t4([1], range(4)), _t4([0], range(4))),
    (_t1([5], [1, 2]) + _t1([6], [0, 1]), _t2(2, range(4))),
    (_t2(2, range(4, 8)), _t4([2], range(4))),
    (_t4([2], [4, 5]) + _t4([0, 1], [5]), _t4([0, 1, 2], [6]) + _t4([0], [4])),
    (_t1([6], [2]) + _t1([7], [0, 1, 2]), _t4([0, 1, 2], [7]) + _t4([1], [4])),
    (_t2(3, [1, 2, 3, 4]), _t2(3, [5, 6, 7]) + _t4([3], [0])),
    (_t4([3], [1, 2, 3, 4]), _t4([3], [5, 6, 7]) + _t2(3, [0])),
]
_A_TAIL = [
    (_t3([0]) + _t3([2], [0]), _t3([1], [0, 1]) + _t3([7], [0])),
    (_t3([2], [1, 2, 3]) + _t3([3], [2, 3]), _t3([1], [2, 3]) + _t3([7], [1])),
    (_t3([4], [0, 1, 3]) + _t3([5], [0, 1]), _t3([3], [0, 1]) + _t3([7], [2])),
    (_t3([5], [2]) + _t3([6]), _t3([4], [2]) + _t3([5], [3]) + _t3([7], [3])),
]
N_T1 = 5
NIT = len(_Q_MAIN)
N_R = len(_A_TAIL)
T_SWO = 7


def _qbuf():
    buf = {}
    for it in _Q_MAIN:
        for b in (0, 1):
            for u in it[b]:
                buf[u] = b
    for u in _Q_TAIL:
        buf[u] = 0
    for it in _A_MAIN + _A_TAIL:
        for b in (0, 1):
            for u in it[b]:
                if u in _Q_PRO:
                    buf[u] = 1 - b
    done = set(_Q_PRO)
    att = set()
    for (qa, qb), (aa, ab) in zip(_Q_MAIN, _A_MAIN):
        assert len(qa) == len(qb) == len(aa) == len(ab) == 4
        assert all(u in done and buf[u] == 1 for u in aa), (qa, aa)
        done |= set(qa)
        assert all(u in done and buf[u] == 0 for u in ab), (qa, ab)
        done |= set(qb)
        att |= set(aa) | set(ab)
    assert all(u in att for u in range(64, 128))
    for (aa, ab), u0 in zip(_A_TAIL, _Q_TAIL):
        done.add(u0)
        assert len(aa) == N_T1 and len(ab) == 8 - N_T1
        assert all(u in done and buf[u] == 1 for u in aa)
        assert all(u in done and buf[u] == 0 for u in ab)
        att |= set(aa) | set(ab)
    assert done == set(range(128)) and att == set(range(128))
    n_q = len(_Q_PRO) + sum(len(a) + len(b) for a, b in _Q_MAIN) + len(_Q_TAIL)
    n_a = sum(len(a) + len(b) for a, b in _A_MAIN + _A_TAIL)
    assert n_q == 128 and n_a == 128
    return buf


_QBUF = _qbuf()


def _wait_slots(need, nslots):
    n = len(need)
    slots = [[] for _ in range(n)]
    pending = []
    for t in range(n - 1, -1, -1):
        pending = sorted(need[t]) + pending
        take = pending[-nslots:]
        pending = pending[:-nslots] if len(pending) > nslots else []
        slots[t] = take
    assert not pending
    return [s + [-1] * (nslots - len(s)) for s in slots]


def _first_need(lists, key):
    seen, need = set(), []
    for a, b in lists:
        cur = {key(u) for u in a + b if key(u) is not None} - seen
        seen |= cur
        need.append(cur)
    return need


_WX = _wait_slots(_first_need(_Q_MAIN, lambda u: (u & 3) if u >= 64 else None), 1)
_WW = _wait_slots(
    _first_need(_Q_MAIN, lambda u: ((u >> 2) & 15) - 8 if ((u >> 2) & 15) >= 8 else None), 2)
_WKV = _wait_slots(_first_need(_A_MAIN, lambda u: (u >> 2) & 15), 3)

_QOFF = 0
_AOFF = _QOFF + 8 * NIT
_TOFF = _AOFF + 8 * NIT
_WOFF = _TOFF + 9 * len(_A_TAIL)
_TABN = _WOFF + 6 * NIT


def _body(x_hbm, wq_hbm, k_hbm, v_hbm, wo_hbm, out_ref,
          xf, wqf, wof, kvf, xb, wqb, wob, q0, q1, ctx, psend, precv,
          tab, sem_x, sem_wq, sem_kv, sem_wo,
          send, xs_recv, wq_recv, wo_recv, p_recv):
    p = lax.axis_index("i")
    r = p ^ 1
    h = 3 - p

    bar = pltpu.get_barrier_semaphore()
    pl.semaphore_signal(bar, inc=1, device_id=(r,), device_id_type=MESH)
    pl.semaphore_signal(bar, inc=1, device_id=(h,), device_id_type=MESH)

    def cols(j):
        return pl.ds(pl.multiple_of(j * 128, 128), 128)

    def ld_x(c):
        return pltpu.make_async_copy(x_hbm.at[:, c], xf.at[c], sem_x.at[c])

    def ld_wq(k):
        return pltpu.make_async_copy(wq_hbm.at[:, cols(k)], wqf.at[k], sem_wq.at[k])

    def ld_k(k16, g, k):
        return pltpu.make_async_copy(k_hbm.at[:, :, :, g, k, :], kvf.at[k16, 0], sem_kv.at[k16])

    def ld_v(k16, g, k):
        return pltpu.make_async_copy(v_hbm.at[:, :, :, g, k, :], kvf.at[k16, 1], sem_kv.at[k16])

    def ld_wo(j):
        return pltpu.make_async_copy(wo_hbm.at[:, cols(j)], wof.at[j], sem_wo.at[j])

    def rc_x(c):
        return pltpu.make_async_remote_copy(
            xb.at[0, c], xb.at[1, c], send.at[0], xs_recv.at[c],
            device_id=(r,), device_id_type=MESH)

    def rc_wq(k):
        return pltpu.make_async_remote_copy(
            wqb.at[k], wqb.at[8 + k], send.at[1], wq_recv.at[k],
            device_id=(h,), device_id_type=MESH)

    def rc_wo(j):
        return pltpu.make_async_remote_copy(
            wob.at[j, pl.ds(0, 1024)], wob.at[j, pl.ds(1024, 1024)],
            send.at[2], wo_recv.at[j], device_id=(h,), device_id_type=MESH)

    def rc_p(j):
        return pltpu.make_async_remote_copy(
            psend.at[j], precv.at[j], send.at[3], p_recv.at[j],
            device_id=(r,), device_id_type=MESH)

    def issue_xw(i, carry):
        nx, nw = carry
        is_x = ((_X_SLOTS >> i) & 1) == 1

        @pl.when(is_x)
        def _():
            ld_x(nx).start()

        @pl.when(jnp.logical_not(is_x))
        def _():
            ld_wq(nw).start()

        d = is_x.astype(jnp.int32)
        return nx + d, nw + 1 - d

    lax.fori_loop(0, 12, issue_xw, (0, 0))

    def issue_kv(i, carry):
        g = jnp.where(i < 8, p, h)
        ld_k(i, g, i & 7).start()
        ld_v(i, g, i & 7).start()
        return carry

    lax.fori_loop(0, 2, issue_kv, 0)

    for t in range(NIT):
        for j, u in enumerate(_Q_MAIN[t][0] + _Q_MAIN[t][1]):
            tab[_QOFF + 8 * t + j] = u
        for j, u in enumerate(_A_MAIN[t][0] + _A_MAIN[t][1]):
            tab[_AOFF + 8 * t + j] = u
        for j, w in enumerate(_WX[t] + _WW[t] + _WKV[t]):
            tab[_WOFF + 6 * t + j] = w
    for t in range(len(_A_TAIL)):
        for j, u in enumerate(_A_TAIL[t][0] + _A_TAIL[t][1] + [_Q_TAIL[t]]):
            tab[_TOFF + 9 * t + j] = u

    def dec(code):
        return code >> 6, (code >> 2) & 15, code & 3

    def QU(code, qbuf):
        s, k, c = dec(code)
        q = jnp.dot(xb[s, c], wqb[k], preferred_element_type=f32)
        qbuf[code] = (q * (SCALE * LOG2E)).astype(bf16)

    def S(code, qbuf):
        s, k, c = dec(code)
        kc = kvf[k, 0, :, c].reshape(256, 128).astype(bf16)
        return lax.dot_general(qbuf[code], kc, _NT, preferred_element_type=f32)

    def softmax(s):
        m = jnp.max(s, axis=-1, keepdims=True)
        e = jnp.exp2(s - m)
        l = jnp.sum(e, axis=-1, keepdims=True)
        return (e * pl.reciprocal(l, approx=False, full_range=False)).astype(bf16)

    def PV(code, probs):
        s, k, c = dec(code)
        vc = kvf[k, 1, :, c].reshape(256, 128).astype(bf16)
        o = jnp.dot(probs, vc, preferred_element_type=f32)
        ctx[s, :, c, :, cols(k)] = o.astype(bf16).reshape(4, 64, 128)

    def conv_x(c):
        xb[0, c] = xf[c].reshape(256, 1024).astype(bf16)

    def conv_wq(k):
        wqb[k] = wqf[k].astype(bf16)

    def QP(k, c):
        u = _code(0, k, c)
        QU(u, (q0, q1)[_QBUF[u]])

    ld_x(0).wait()
    conv_x(0)
    ld_wq(0).wait()
    conv_wq(0)
    pl.semaphore_wait(bar, 2)
    rc_x(0).start()
    rc_wq(0).start()
    for xs, ws, units in _STAGES:
        if xs == [2]:
            lax.fori_loop(2, 16, issue_kv, 0)
        for c in xs:
            ld_x(c).wait()
        for k in ws:
            ld_wq(k).wait()
        for c in xs:
            conv_x(c)
        for k in ws:
            conv_wq(k)
        for k, c in units:
            QP(k, c)
        for c in xs:
            rc_x(c).start()
        for k in ws:
            rc_wq(k).start()

    for j in range(8):
        ld_wo(j).start()

    def wait_kv(i):
        pltpu.make_async_copy(kvf.at[i], kvf.at[i], sem_kv.at[i]).wait()

    def step(A, Q, qr, qw):
        QU(Q[0], qw)
        Ss = [S(a, qr) for a in A[:2]]
        QU(Q[1], qw)
        Ss += [S(a, qr) for a in A[2:]]
        QU(Q[2], qw)
        E = [softmax(s) for s in Ss]
        PV(A[0], E[0])
        PV(A[1], E[1])
        PV(A[2], E[2])
        PV(A[3], E[3])
        QU(Q[3], qw)

    def do_main(t, carry):
        w = [tab[_WOFF + 6 * t + j] for j in range(6)]
        pl.when(w[0] >= 0)(lambda: rc_x(w[0]).wait_recv())
        for j in (1, 2):
            pl.when(w[j] >= 0)(lambda j=j: rc_wq(w[j]).wait_recv())
        for j in (3, 4, 5):
            pl.when(w[j] >= 0)(lambda j=j: wait_kv(w[j]))

        @pl.when(t == T_SWO)
        def _():
            for j in range(8):
                ld_wo(j).wait()
            for j in range(8):
                wob[j, 0:1024, :] = wof[j].astype(bf16)
            for j in range(8):
                rc_wo(j).start()

        A = [tab[_AOFF + 8 * t + j] for j in range(8)]
        Q = [tab[_QOFF + 8 * t + j] for j in range(8)]
        step(A[:4], Q[:4], q1, q0)
        step(A[4:], Q[4:], q0, q1)
        return carry

    def o_remote(j):
        lhs = ctx[1].reshape(1024, 2048)
        psend[j] = jnp.dot(lhs, wob[j], preferred_element_type=f32).astype(bf16)

    def o_local(j, add):
        lhs = ctx[0].reshape(1024, 2048)
        res = jnp.dot(lhs, wob[j], preferred_element_type=f32)
        out_ref[0, :, cols(j)] = res + add

    def do_r(j, carry):
        pl.when(j > 0)(lambda: rc_p(j - 1).start())
        rc_wo(j).wait_recv()
        A = [tab[_TOFF + 9 * j + i] for i in range(9)]
        QU(A[8], q0)
        Ss = [S(a, q1) for a in A[:N_T1]] + [S(a, q0) for a in A[N_T1:8]]
        o_remote(j)
        E = [softmax(s) for s in Ss]
        for a, e in zip(A[:8], E):
            PV(a, e)
        return carry

    lax.fori_loop(0, NIT, do_main, 0)
    lax.fori_loop(0, N_R, do_r, 0)
    rc_p(N_R - 1).start()
    NX = N_R

    def do_rp(j, carry):
        pl.when(j > NX)(lambda: rc_p(j - 1).start())
        rc_wo(j).wait_recv()
        rc_p(j - NX).wait_recv()
        o_local(j - NX, precv[j - NX].astype(f32))
        o_remote(j)
        return carry

    lax.fori_loop(NX, 8, do_rp, 0)
    rc_p(7).start()

    def do_pp(i, carry):
        j = 4 + 2 * i
        first = i == 0
        rc_p(j).wait_recv()
        pl.when(first)(lambda: rc_p(5).wait_recv())
        o_local(j, precv[j].astype(f32))
        o_local(j + 1, jnp.where(first, precv[jnp.where(first, 5, 4)].astype(f32), 0.0))
        return carry

    lax.fori_loop(0, 2, do_pp, 0)
    rc_p(7).wait_recv()
    out_ref[0, :, cols(7)] = out_ref[0, :, cols(7)] + precv[7].astype(f32)

    def wait_sent(src, dst, i, recv_sem, dev):
        pltpu.make_async_remote_copy(src, dst, send.at[i], recv_sem, device_id=(dev,),
                                     device_id_type=MESH).wait_send()

    wait_sent(xb.at[0], xb.at[1], 0, xs_recv.at[0], r)
    wait_sent(wqb.at[pl.ds(0, 8)], wqb.at[pl.ds(8, 8)], 1, wq_recv.at[0], h)
    wait_sent(wob.at[:, pl.ds(0, 1024)], wob.at[:, pl.ds(1024, 1024)], 2, wo_recv.at[0], h)
    wait_sent(psend, precv, 3, p_recv.at[0], r)


_X_SLOTS = (1 << 0) | (1 << 3) | (1 << 6) | (1 << 11)


def pallas_dist_sparse_attn_strided_qseq_b1_sq1024_skv1024_hq8_dh128_kernel(
    x: jax.Array,
    Wq: jax.Array,
    K_ext: jax.Array,
    V_ext: jax.Array,
    Wo: jax.Array,
):
    x4 = x.reshape(4, 4, 64, 1024)
    k6 = K_ext.reshape(4, 4, 64, 4, 8, 128)
    v6 = V_ext.reshape(4, 4, 64, 4, 8, 128)
    DMA = pltpu.SemaphoreType.DMA
    return pl.pallas_call(
        _body,
        out_shape=jax.ShapeDtypeStruct((1, 1024, 1024), f32),
        in_specs=[pl.BlockSpec(memory_space=pl.ANY)] * 5,
        out_specs=pl.BlockSpec(memory_space=pltpu.VMEM),
        scratch_shapes=[
            pltpu.VMEM((4, 4, 64, 1024), f32),
            pltpu.VMEM((8, 1024, 128), f32),
            pltpu.VMEM((8, 1024, 128), f32),
            pltpu.VMEM((16, 2, 4, 4, 64, 128), f32),
            pltpu.VMEM((2, 4, 256, 1024), bf16),
            pltpu.VMEM((16, 1024, 128), bf16),
            pltpu.VMEM((8, 2048, 128), bf16),
            pltpu.VMEM((128, 256, 128), bf16),
            pltpu.VMEM((128, 256, 128), bf16),
            pltpu.VMEM((2, 4, 4, 64, 2048), bf16),
            pltpu.VMEM((8, 1024, 128), bf16),
            pltpu.VMEM((8, 1024, 128), bf16),
            pltpu.SMEM((_TABN,), jnp.int32),
            DMA((4,)), DMA((8,)), DMA((16,)), DMA((8,)),
            DMA((4,)), DMA((4,)), DMA((8,)), DMA((8,)), DMA((8,)),
        ],
        compiler_params=pltpu.CompilerParams(
            collective_id=0, vmem_limit_bytes=96 * 1024 * 1024,
            disable_bounds_checks=True, disable_semaphore_checks=True),
    )(x4, Wq, k6, v6, Wo)
```
